```python
import numpy as np

kernel_name = "dist_mlp2_tp_i_m512_h1024_out512"

def setup_inputs():
    x = np.random.randn(512, 512).astype(np.float32)
    W1 = np.random.randn(512, 4096).astype(np.float32)
    W2 = np.random.randn(4096, 512).astype(np.float32)
    return {"x": x, "W1": W1, "W2": W2}

def reference(x: np.ndarray, W1: np.ndarray, W2: np.ndarray) -> np.ndarray:
    h = x @ W1
    h = np.maximum(h, 0.0)
    return h @ W2
```

```python
import contextlib
import jax
import jax.numpy as jnp
from jax import lax
from jax.experimental import pallas as pl
from jax.experimental.pallas import tpu as pltpu

BF = jnp.bfloat16
F32 = jnp.float32
ds = pl.ds
MESH = pl.DeviceIdType.MESH
B = 128


def pallas_dist_mlp2_tp_i_m512_h1024_out512_kernel(x, W1, W2):
    use_scopes = False
    M, K = x.shape
    H = W1.shape[1]
    N = W2.shape[1]
    NC = N // B
    NK = K // B

    def body(x_ref, w1_ref, w2_ref, o_ref,
             xb, w1b, w2b, xh, hacc, hb, own, s1, r1, s2, r2, s3, r3,
             ld_sem, send_sem, recv_sem):
        sc = (lambda n: jax.named_scope(n)) if use_scopes else (lambda n: contextlib.nullcontext())
        me = lax.axis_index("i")
        a = me >> 1
        b = ((me + 1) >> 1) & 1
        nbrP = me ^ 1
        nbrQ = 3 - me
        gblk = [1 - a, 3 - b, a, 2 + b]
        nb13 = [nbrQ, nbrP]
        nb2 = [nbrP, nbrQ]

        bs = pltpu.get_barrier_semaphore()
        for nbr in (nbrP, nbrQ):
            pl.semaphore_signal(bs, inc=1, device_id=(nbr,), device_id_type=MESH)

        cx = [pltpu.make_async_copy(x_ref.at[ds(pl.multiple_of(gblk[i] * B, B), B)], xb.at[ds(i * B, B)], ld_sem.at[i]) for i in range(4)]
        c1 = [pltpu.make_async_copy(w1_ref.at[ds(B * k, B)], w1b.at[ds(B * k, B)], ld_sem.at[4 + k]) for k in range(NK)]
        c2 = [pltpu.make_async_copy(w2_ref.at[:, ds(B * j, B)], w2b.at[j], ld_sem.at[8 + j]) for j in range(NC)]
        for c in (cx[0], cx[1], c1[0], cx[2], cx[3], c1[1], c1[2], c1[3], *c2):
            c.start()

        def rdma(ph, l, j):
            src = (s1, s2, s3)[ph]
            dst = (r1, r2, r3)[ph]
            tgt = nb2[l] if ph == 1 else nb13[l]
            i = ph * 2 * NC + l * NC + j
            return pltpu.make_async_remote_copy(src.at[l, j], dst.at[l, j], send_sem.at[i], recv_sem.at[i],
                                                device_id=(tgt,), device_id_type=MESH)

        def hstep(k, rows):
            w = w1b[ds(B * k, B), :].astype(BF)
            p = jnp.dot(xh[rows, ds(B * k, B)], w, preferred_element_type=F32)
            if k == 0:
                hacc[rows, :] = p
            elif k < NK - 1:
                hacc[rows, :] += p
            else:
                hb[rows, :] = jnp.maximum(hacc[rows, :] + p, 0).astype(BF)

        LEAF = ds(0, 2 * B)
        ROOT = ds(2 * B, 2 * B)
        ALL = ds(0, 4 * B)

        with sc("xl"):
            cx[0].wait(); cx[1].wait()
            xh[LEAF, :] = xb[LEAF, :].astype(BF)
        with sc("k0l"):
            c1[0].wait()
            hstep(0, LEAF)
        with sc("k0r"):
            cx[2].wait(); cx[3].wait()
            xh[ROOT, :] = xb[ROOT, :].astype(BF)
            hstep(0, ROOT)
        with sc("k1"):
            c1[1].wait()
            hstep(1, ALL)
        with sc("k2"):
            c1[2].wait()
            hstep(2, ALL)
        with sc("k3l"):
            c1[3].wait()
            hstep(3, LEAF)
        with sc("bar"):
            pl.semaphore_wait(bs, 2)

        def leaf(j):
            w = w2b[j].astype(BF)
            p = jnp.dot(hb[LEAF, :], w, preferred_element_type=F32).astype(BF)
            s1[0, j] = p[:B]
            s1[1, j] = p[B:]
            rdma(0, 0, j).start()
            rdma(0, 1, j).start()

        def root(j):
            w = w2b[j].astype(BF)
            p = jnp.dot(hb[ROOT, :], w, preferred_element_type=F32)
            own[0, j] = p[:B]
            own[1, j] = p[B:]

        def ph2(j):
            for l in range(2):
                rdma(0, l, j).wait_recv()
                s = own[l, j] + r1[l, j].astype(F32)
                own[l, j] = s
                s2[l, j] = s.astype(BF)
                rdma(1, l, j).start()

        def ph3(j):
            for l in range(2):
                rdma(1, l, j).wait_recv()
                t = own[l, j] + r2[l, j].astype(F32)
                s3[l, j] = t.astype(BF)
                rdma(2, l, j).start()
                o_ref[ds(pl.multiple_of(gblk[2 + l] * B, B), B), ds(B * j, B)] = t

        def fin(j):
            for l in range(2):
                rdma(2, l, j).wait_recv()
                o_ref[ds(pl.multiple_of(gblk[l] * B, B), B), ds(B * j, B)] = r3[l, j].astype(F32)

        with sc("L0"):
            c2[0].wait(); leaf(0)
        with sc("k3r"):
            hstep(3, ROOT)
        with sc("L1"):
            c2[1].wait(); leaf(1)
        with sc("R0"):
            root(0)
        with sc("L2"):
            c2[2].wait(); leaf(2)
        with sc("R1"):
            root(1)
        with sc("p2_0"):
            ph2(0)
        with sc("L3"):
            c2[3].wait(); leaf(3)
        with sc("p2_1"):
            ph2(1)
        with sc("R2"):
            root(2)
        with sc("p2_2"):
            ph2(2)
        with sc("R3"):
            root(3)
        for name, f, j in [("p3_0", ph3, 0), ("p2_3", ph2, 3), ("p3_1", ph3, 1), ("p3_2", ph3, 2), ("f0", fin, 0),
                           ("p3_3", ph3, 3), ("f1", fin, 1), ("f2", fin, 2), ("f3", fin, 3)]:
            with sc(name):
                f(j)
        with sc("ws"):
            for ph in range(3):
                for l in range(2):
                    for j in range(NC):
                        rdma(ph, l, j).wait_send()

    cb = lambda: pltpu.VMEM((2, NC, B, B), BF)
    return pl.pallas_call(
        body,
        out_shape=jax.ShapeDtypeStruct((M, N), F32),
        in_specs=[pl.BlockSpec(memory_space=pl.ANY)] * 3,
        out_specs=pl.BlockSpec(memory_space=pltpu.VMEM),
        scratch_shapes=[
            pltpu.VMEM((M, K), F32), pltpu.VMEM((K, H), F32), pltpu.VMEM((NC, H, B), F32),
            pltpu.VMEM((M, K), BF), pltpu.VMEM((M, H), F32), pltpu.VMEM((M, H), BF),
            pltpu.VMEM((2, NC, B, B), F32),
            cb(), cb(), cb(), cb(), cb(), cb(),
            pltpu.SemaphoreType.DMA((12,)),
            pltpu.SemaphoreType.DMA((6 * NC,)),
            pltpu.SemaphoreType.DMA((6 * NC,)),
        ],
        compiler_params=pltpu.CompilerParams(collective_id=0, disable_semaphore_checks=True),
    )(x, W1, W2)
```

```python
import jax
import jax.numpy as jnp
from jax import lax
from jax.experimental import pallas as pl
from jax.experimental.pallas import tpu as pltpu

BF16 = jnp.bfloat16
F32 = jnp.float32
T = 128
U = 16
ROWS = 512
MESH_INDEX = {"A": 0, "B": 1, "D": 2, "C": 3}
BRIDGE = 112
MIN_REST = 32

_LOAD_ORDER = {
    "A": "x.96.416 k0 k1 k2 k3 c0 c1 c2 c3",
    "B": "x.304.480 k0 k1 k2 k3 c0 c1 c2 c3 x.192.256",
    "D": "x.480.512 x.0.32 x.32.80 x.432.480 k0 k1 k2 k3 c0 c1 c2 x.224.288 c3",
}

_SCHEDULE = {
    "A": """
    L.x.96.416 V.96.416 BAR S.B.x.03.272.288 S.C.x.03.224.240 S.B.x.02.256.272 S.C.x.02.240.256
    S.B.x.03.288.304 S.C.x.03.208.224 S.B.x.01.144.192 S.C.x.01.320.368 S.B.x.12.144.192
    S.C.x.12.320.368 S.B.x.23.256.272 S.C.x.23.240.256 S.B.x.34.256.304 S.C.x.34.208.256
    S.B.x.24.144.192 S.C.x.24.320.368 S.B.x.02.96.144 S.C.x.02.368.416 S.B.x.24.96.144
    S.C.x.24.368.416 L.k0 H.96.416.0.1 L.k1 L.k2 H.96.416.1.3 L.k3 H.96.416.3.4 L.c0
    R.B.x.04.432.480 R.C.x.04.32.80 M.0.144.192 M.0.320.368 P.B.p1.0.144.192 P.C.p1.0.320.368
    M.0.192.208 M.0.304.320 M.0.208.304 P.B.p1.0.192.256 P.C.p1.0.256.320 H.48.80.0.4 H.432.464.0.4
    L.c1 R.B.x.04.416.432 R.C.x.04.80.96 M.1.144.192 M.1.320.368 P.B.p1.1.144.192 P.C.p1.1.320.368
    M.1.208.224 M.1.288.304 M.1.240.272 M.1.192.208 M.1.304.320 M.1.224.240 M.1.272.288 H.80.96.0.4
    H.416.432.0.4 S.B.p1.1.192.256 S.C.p1.1.256.320 L.c2 M.2.64.144 M.2.368.448 P.B.p1.2.96.144
    P.C.p1.2.368.416 M.2.48.64 M.2.448.464 M.2.160.352 S.B.p1.2.192.256 S.C.p1.2.256.320 M.2.144.160
    M.2.352.368 S.B.p1.2.144.192 S.C.p1.2.320.368 S.B.p1.2.48.96 S.C.p1.2.416.464 L.c3
    R.B.x.04.480.512 R.C.x.04.0.32 M.3.64.448 P.B.p1.3.64.160 P.C.p1.3.352.448 P.B.p1.3.160.256
    P.C.p1.3.256.352 H.0.48.0.4 H.464.512.0.4 M.1.0.144 M.1.368.512 R.C.p1.1.0.48 R.C.p1.1.48.80
    R.C.p1.1.80.144 S.B.p2.1.32.144 R.B.p1.0.464.512 R.B.p1.0.368.416 R.B.p1.0.416.464
    R.B.p1.1.464.512 R.B.p1.1.432.464 R.B.p1.1.368.432 R.C.p1.0.0.48 R.C.p1.0.96.144 R.C.p1.0.48.96
    S.C.p2.1.368.480 M.3.0.64 M.3.448.512 M.0.0.144 M.0.368.512 P.B.p2.0.80.144 P.C.p2.0.368.432
    M.2.0.48 M.2.464.512 R.C.p2.0.448.512 R.C.p2.0.400.448 S.B.p3.0.432.512 S.B.p1.3.0.64
    R.B.p2.0.0.64 R.B.p2.0.64.112 S.C.p3.0.0.80 S.C.p1.3.448.512 W.B.x.03.272.288 W.C.x.03.224.240
    W.B.x.02.256.272 W.C.x.02.240.256 W.B.x.03.288.304 W.C.x.03.208.224 W.B.x.01.144.192
    W.C.x.01.320.368 W.B.x.12.144.192 W.C.x.12.320.368 R.C.p2.1.464.512 S.B.p3.1.480.512
    S.B.p2.0.48.80 R.B.p2.1.0.48 S.C.p3.1.0.32 S.C.p2.0.432.464 W.B.x.23.256.272 W.C.x.23.240.256
    W.B.x.34.256.304 W.C.x.34.208.256 W.B.x.24.144.192 W.C.x.24.320.368 W.B.x.02.96.144
    W.C.x.02.368.416 W.B.x.24.96.144 W.C.x.24.368.416 R.C.p2.1.400.464 S.B.p3.1.400.480
    R.B.p2.1.48.112 S.C.p3.1.32.112 R.C.p1.2.0.48 S.B.p2.2.0.48 R.B.p1.2.464.512 S.C.p2.2.464.512
    R.C.p2.0.368.400 S.B.p3.0.368.400 R.B.p2.0.112.144 S.C.p3.0.112.144 R.C.p2.1.368.400
    S.B.p3.1.368.400 S.B.p3.0.400.432 S.B.p2.0.0.48 R.B.p2.1.112.144 S.C.p3.1.112.144
    S.C.p3.0.80.112 S.C.p2.0.464.512 W.B.p1.0.144.192 W.C.p1.0.320.368 W.B.p1.0.192.256
    W.C.p1.0.256.320 W.B.p1.1.144.192 W.C.p1.1.320.368 W.B.p1.1.192.256 W.C.p1.1.256.320
    W.B.p1.2.96.144 W.C.p1.2.368.416 R.B.p3.0.144.192 F.B.p3.0.144.192 R.C.p3.0.320.368
    F.C.p3.0.320.368 W.B.p1.2.192.256 W.C.p1.2.256.320 W.B.p1.2.144.192 W.C.p1.2.320.368
    W.B.p1.2.48.96 W.C.p1.2.416.464 W.B.p1.3.64.160 W.C.p1.3.352.448 W.B.p1.3.160.256
    W.C.p1.3.256.352 R.B.p3.1.144.192 F.B.p3.1.144.192 R.C.p3.1.320.368 F.C.p3.1.320.368
    W.B.p2.1.32.144 W.C.p2.1.368.480 W.B.p2.0.80.144 W.C.p2.0.368.432 W.B.p3.0.432.512 W.B.p1.3.0.64
    W.C.p3.0.0.80 W.C.p1.3.448.512 R.B.p3.0.192.224 F.B.p3.0.192.224 R.C.p3.0.288.320
    F.C.p3.0.288.320 W.B.p3.1.480.512 W.C.p3.1.0.32 R.B.p3.1.192.224 F.B.p3.1.192.224
    R.C.p3.1.288.320 F.C.p3.1.288.320 W.B.p2.0.48.80 W.C.p2.0.432.464 R.B.p3.2.48.96 F.B.p3.2.48.96
    R.C.p3.2.416.464 F.C.p3.2.416.464 R.B.p3.2.96.144 F.B.p3.2.96.144 R.C.p3.2.368.416
    F.C.p3.2.368.416 W.B.p3.1.400.480 W.C.p3.1.32.112 R.C.p3.0.256.288 S.B.fw.0.256.320
    S.B.p2.1.0.32 R.B.p3.0.224.256 S.C.fw.0.192.256 S.C.p2.1.480.512 R.C.p2.2.464.512
    S.B.p3.2.464.512 R.B.p2.2.0.48 S.C.p3.2.0.48 F.B.p3.0.224.256 F.C.p3.0.256.288 R.C.p3.1.256.288
    S.B.fw.1.256.320 S.B.fw.2.384.464 R.B.p3.1.224.256 S.C.fw.1.192.256 S.C.fw.2.48.128
    F.B.p3.1.224.256 F.C.p3.1.256.288 W.B.p2.2.0.48 W.C.p2.2.464.512 W.B.p3.0.368.400
    W.C.p3.0.112.144 R.B.p3.2.192.224 F.B.p3.2.192.224 R.C.p3.2.288.320 F.C.p3.2.288.320
    W.B.p3.1.368.400 W.C.p3.1.112.144 R.B.p3.2.224.256 F.B.p3.2.224.256 R.C.p3.2.256.288
    F.C.p3.2.256.288 W.B.p3.0.400.432 W.C.p3.0.80.112 R.B.p3.2.144.192 F.B.p3.2.144.192
    R.C.p3.2.320.368 F.C.p3.2.320.368 W.B.p2.0.0.48 W.C.p2.0.464.512 R.B.p3.3.32.80 F.B.p3.3.32.80
    R.C.p3.3.432.480 F.C.p3.3.432.480 W.B.fw.0.256.320 W.C.fw.0.192.256 R.B.p3.3.0.32 F.B.p3.3.0.32
    R.C.p3.3.480.512 F.C.p3.3.480.512 W.B.p2.1.0.32 R.B.p3.3.128.176 F.B.p3.3.128.176
    R.C.p3.3.336.384 F.C.p3.3.336.384 W.C.p2.1.480.512 W.B.p3.2.464.512 W.C.p3.2.0.48
    R.B.p3.3.80.128 F.B.p3.3.80.128 R.C.p3.3.384.432 F.C.p3.3.384.432 R.B.p3.3.208.256
    F.B.p3.3.208.256 R.C.p3.3.256.304 F.C.p3.3.256.304 W.B.fw.1.256.320 W.C.fw.1.192.256
    R.B.p3.3.176.208 F.B.p3.3.176.208 R.C.p3.3.304.336 F.C.p3.3.304.336 W.B.fw.2.384.464
    W.C.fw.2.48.128
    """,
    "B": """
    L.x.304.480 V.304.480 BAR S.A.x.04.432.480 S.D.x.01.368.432 S.D.x.12.368.432 S.D.x.23.368.432
    S.A.x.04.416.432 S.D.x.02.336.368 S.D.x.34.416.432 S.D.x.34.400.416 S.D.x.02.320.336
    S.D.x.34.368.384 S.D.x.34.384.400 S.D.x.24.320.368 L.k0 H.304.480.0.1 L.k1 R.A.x.03.272.288
    R.A.x.02.256.272 R.A.x.03.288.304 H.256.304.0.2 H.304.480.1.2 R.D.x.02.0.32 R.A.x.01.144.192
    R.A.x.12.144.192 R.D.x.03.496.512 H.0.32.0.2 H.144.192.0.2 R.D.x.04.480.496 L.k2
    R.A.x.23.256.272 H.480.512.0.2 H.256.512.2.3 L.k3 R.D.x.23.0.32 R.D.x.34.0.32 R.D.x.34.496.512
    R.A.x.34.256.304 R.A.x.24.144.192 S.A.x.04.480.512 S.D.x.04.288.320 H.0.32.2.4 H.256.512.3.4
    H.144.192.2.4 L.c0 R.D.x.04.32.64 R.A.x.02.96.144 M.0.336.368 M.0.464.512 P.A.p1.0.464.512
    P.D.p1.0.336.368 M.0.256.336 M.0.0.32 P.D.p1.0.256.336 M.0.368.464 P.A.p1.0.368.416
    P.A.p1.0.416.464 H.96.144.0.2 H.32.64.0.2 M.0.144.192 R.A.p1.0.144.192 S.D.p2.0.144.192
    R.D.x.04.64.80 R.D.x.03.80.96 R.A.x.24.96.144 L.c1 M.1.464.512 P.A.p1.1.464.512 M.1.432.464
    M.1.320.384 P.D.p1.1.320.368 P.A.p1.1.432.464 H.64.96.0.1 M.1.384.432 M.1.256.320 H.64.96.1.2
    P.D.p1.1.288.320 P.A.p1.1.368.432 P.D.p1.1.256.288 M.1.144.192 H.32.144.2.3 H.128.144.3.4
    H.32.64.3.4 R.A.p1.1.144.192 S.D.p2.1.144.192 R.D.x.34.80.96 R.A.p1.0.192.256 L.c2 M.2.464.512
    P.A.p1.2.464.512 M.2.368.464 P.D.p1.2.416.464 P.D.p1.2.368.416 H.64.128.3.4 M.0.32.64
    R.D.p1.0.0.32 R.D.p1.0.32.64 S.A.p2.0.0.64 M.2.256.368 M.0.64.144 S.D.p1.2.256.368
    R.D.p1.0.96.144 S.A.p2.0.112.144 R.A.p1.1.192.256 R.A.p1.2.96.144 R.D.p1.0.64.96 S.A.p2.0.64.112
    L.c3 M.3.368.512 M.1.0.64 S.D.p1.3.400.512 R.D.p1.1.0.32 R.D.p1.1.32.64 S.A.p2.1.0.48
    L.x.192.256 R.A.p1.2.192.256 M.1.64.144 V.192.256 R.D.p1.1.64.112 S.A.p2.1.48.112
    R.A.p1.2.144.192 M.2.0.16 M.2.16.48 M.3.256.368 S.D.p1.3.336.400 S.D.p1.3.256.336
    R.D.p1.1.112.144 S.A.p2.1.112.144 R.A.p1.2.48.96 R.D.p2.0.144.192 S.A.p3.0.144.192 H.192.256.0.2
    R.D.p1.2.0.48 S.A.p2.2.0.48 H.192.256.2.4 R.D.p2.1.144.192 S.A.p3.1.144.192 R.A.p1.3.64.160
    M.1.192.224 M.0.192.256 S.D.p2.0.192.256 R.D.p2.0.192.224 S.A.p3.0.192.224 R.D.p2.1.192.224
    S.A.p3.1.192.224 M.2.48.192 S.D.p2.2.128.192 R.D.p2.2.48.96 S.A.p3.2.48.96 R.A.p1.3.160.256
    M.1.224.256 M.2.192.256 S.D.p2.2.192.256 R.D.p2.2.96.144 S.A.p3.2.96.144 M.3.144.256
    S.D.p2.3.224.256 R.D.p2.0.224.256 S.A.p3.0.224.256 R.A.p2.1.32.144 R.D.p2.1.224.256
    S.A.p3.1.224.256 M.3.32.144 S.D.p2.3.128.176 S.D.p2.3.176.224 R.D.p2.2.176.224 S.A.p3.2.192.224
    R.A.p2.0.80.144 M.3.0.32 R.D.p2.2.224.256 S.A.p3.2.224.256 R.A.p3.0.432.512 F.A.p3.0.432.512
    W.A.x.04.432.480 W.D.x.01.368.432 W.D.x.12.368.432 W.D.x.23.368.432 W.A.x.04.416.432
    W.D.x.02.336.368 W.D.x.34.416.432 W.D.x.34.400.416 W.D.x.02.320.336 W.D.x.34.368.384
    R.D.p2.2.144.176 S.A.p3.2.144.192 R.A.p1.3.0.64 S.D.p2.3.0.128 S.D.p3.1.80.144 S.D.p3.1.32.80
    S.D.p2.2.48.128 R.A.p3.1.480.512 F.A.p3.1.480.512 R.D.p2.3.32.80 S.A.p3.3.32.80 W.D.x.34.384.400
    W.D.x.24.320.368 W.A.x.04.480.512 W.D.x.04.288.320 W.A.p1.0.464.512 W.D.p1.0.336.368
    W.D.p1.0.256.336 W.A.p1.0.368.416 W.A.p1.0.416.464 W.D.p2.0.144.192 R.D.p2.3.0.32 S.A.p3.3.0.32
    W.A.p1.1.464.512 W.D.p1.1.320.368 W.A.p1.1.432.464 W.D.p1.1.288.320 W.A.p1.1.368.432
    W.D.p1.1.256.288 W.D.p2.1.144.192 W.A.p1.2.464.512 W.D.p1.2.416.464 W.D.p1.2.368.416
    R.D.p2.3.128.176 S.A.p3.3.128.176 R.A.p3.1.400.480 F.A.p3.1.400.480 W.A.p2.0.0.64
    W.D.p1.2.256.368 W.A.p2.0.112.144 W.A.p2.0.64.112 W.D.p1.3.400.512 W.A.p2.1.0.48 W.A.p2.1.48.112
    W.D.p1.3.336.400 W.D.p1.3.256.336 W.A.p2.1.112.144 R.D.p2.3.80.128 S.A.p3.3.80.128 R.A.p2.2.0.48
    S.D.p3.2.0.48 W.A.p3.0.144.192 W.A.p2.2.0.48 W.A.p3.1.144.192 W.D.p2.0.192.256 W.A.p3.0.192.224
    W.A.p3.1.192.224 W.D.p2.2.128.192 W.A.p3.2.48.96 W.D.p2.2.192.256 W.A.p3.2.96.144
    R.D.p2.3.208.256 S.A.p3.3.208.256 R.A.p3.0.368.400 F.A.p3.0.368.400 W.D.p2.3.224.256
    W.A.p3.0.224.256 W.A.p3.1.224.256 W.D.p2.3.128.176 W.D.p2.3.176.224 W.A.p3.2.192.224
    W.A.p3.2.224.256 W.A.p3.2.144.192 W.A.p3.3.32.80 R.D.p2.3.176.208 S.A.p3.3.176.208
    R.A.p3.1.368.400 F.A.p3.1.368.400 W.A.p3.3.0.32 R.A.p3.0.400.432 F.A.p3.0.400.432
    R.D.p3.0.320.368 F.D.p3.0.320.368 R.A.p2.0.48.80 W.D.p2.3.0.128 W.A.p3.3.128.176 R.A.p2.0.0.48
    S.D.p3.0.32.112 R.D.p3.1.320.368 F.D.p3.1.320.368 W.D.p3.1.80.144 W.A.p3.3.80.128
    R.A.fw.0.256.320 F.A.fw.0.256.320 W.D.p3.1.32.80 W.A.p3.3.208.256 R.A.p2.1.0.32 S.D.p3.1.0.32
    S.D.p2.1.192.256 S.D.p3.0.112.144 S.D.p3.0.0.32 W.A.p3.3.176.208 R.D.p3.2.256.384
    F.D.p3.2.256.384 R.A.p3.2.464.512 F.A.p3.2.464.512 W.D.p2.2.48.128 R.A.fw.1.256.320
    F.A.fw.1.256.320 R.D.p3.3.256.336 F.D.p3.3.256.336 W.D.p3.2.0.48 R.D.p3.3.336.384
    F.D.p3.3.336.384 R.A.fw.2.384.464 F.A.fw.2.384.464 R.D.p3.3.384.416 F.D.p3.3.384.416
    W.D.p3.0.32.112 W.D.p3.1.0.32 R.D.p3.3.464.512 F.D.p3.3.464.512 R.D.p3.3.416.464
    F.D.p3.3.416.464 W.D.p2.1.192.256 W.D.p3.0.112.144 W.D.p3.0.0.32
    """,
    "D": """
    L.x.480.512 BAR V.480.512 S.B.x.03.496.512 L.x.0.32 V.0.32 S.C.x.03.0.16 S.B.x.02.0.32
    S.C.x.02.480.512 S.B.x.04.480.496 S.C.x.04.16.32 S.B.x.23.0.32 S.C.x.23.480.512 S.B.x.34.0.32
    S.C.x.34.480.512 S.B.x.34.496.512 S.C.x.34.0.16 L.x.32.80 V.32.80 S.B.x.04.32.64 S.B.x.04.64.80
    L.x.432.480 V.432.480 S.C.x.04.448.480 S.C.x.04.432.448 L.k0 R.B.x.01.368.432 R.C.x.01.80.144
    H.0.144.0.1 H.368.512.0.1 L.k1 R.B.x.12.368.432 R.C.x.12.80.144 H.0.144.1.2 H.368.512.1.2 L.k2
    R.B.x.23.368.432 R.B.x.02.336.368 R.C.x.23.80.144 R.C.x.02.144.176 S.B.x.03.80.96
    S.C.x.03.416.432 H.144.176.0.1 H.336.368.0.1 H.144.160.1.2 H.352.368.1.2 H.160.176.1.2
    H.336.352.1.2 H.0.144.2.3 H.368.512.2.3 L.k3 R.B.x.34.416.432 R.B.x.34.400.416 R.B.x.34.368.384
    R.B.x.34.384.400 R.C.x.34.80.96 R.C.x.34.96.112 R.C.x.34.128.144 R.C.x.34.112.128
    R.B.x.02.320.336 R.C.x.02.176.192 S.B.x.34.80.96 S.C.x.34.416.432 H.0.144.3.4 H.368.512.3.4
    H.176.192.0.2 H.320.336.0.2 L.c0 R.B.x.24.320.368 R.C.x.24.144.192 M.0.0.32 M.0.480.512
    P.B.p1.0.0.32 P.C.p1.0.480.512 M.0.32.80 M.0.432.480 P.B.p1.0.32.64 P.C.p1.0.448.480 M.0.80.144
    M.0.368.432 P.B.p1.0.96.144 P.C.p1.0.368.416 P.B.p1.0.64.96 P.C.p1.0.416.448 H.144.192.2.4
    H.320.368.2.4 L.c1 R.B.x.04.288.320 R.C.x.04.192.224 M.1.0.32 M.1.480.512 P.B.p1.1.0.32
    P.C.p1.1.480.512 M.1.32.80 M.1.432.480 P.B.p1.1.32.64 P.C.p1.1.448.480 M.1.80.144 M.1.368.432
    P.B.p1.1.64.112 P.C.p1.1.400.448 P.B.p1.1.112.144 P.C.p1.1.368.400 H.192.224.0.4 H.288.320.0.4
    M.0.144.192 M.0.320.368 R.C.p1.0.144.176 R.C.p1.0.176.256 S.B.p2.0.144.192 R.B.p1.0.336.368
    R.B.p1.0.256.336 S.C.p2.0.320.368 L.c2 M.2.0.48 M.2.464.512 P.B.p1.2.0.48 P.C.p1.2.464.512
    M.1.144.224 M.1.288.368 R.C.p1.1.144.192 S.B.p2.1.144.192 L.x.224.288 R.B.p2.0.144.192
    R.B.p1.1.320.368 R.B.p1.1.288.320 R.C.p2.0.320.368 R.C.p1.1.192.224 S.C.p2.1.320.368 V.224.288
    M.0.192.224 M.0.288.320 P.B.p2.0.192.224 P.C.p2.0.288.320 P.B.p2.1.192.224 P.C.p2.1.288.320
    H.224.288.0.4 M.2.48.96 M.2.416.464 R.C.p1.2.48.96 S.B.p2.2.48.96 L.c3 R.B.p1.1.256.288
    R.B.p2.1.144.192 R.B.p1.2.416.464 R.C.p1.1.224.256 R.C.p2.1.320.368 S.C.p2.2.416.464 M.2.96.144
    M.2.368.416 R.C.p1.2.96.144 S.B.p2.2.96.144 R.B.p1.2.368.416 S.C.p2.2.368.416 M.0.224.288
    P.B.p2.0.224.256 P.C.p2.0.256.288 M.2.144.160 M.2.352.368 M.1.224.288 P.B.p2.1.224.256
    P.C.p2.1.256.288 M.2.224.288 M.2.208.224 M.2.288.304 M.2.160.208 M.2.304.352 R.C.p1.2.144.256
    S.B.p2.2.176.224 R.B.p1.2.256.368 S.C.p2.2.288.336 S.B.p2.2.224.256 S.C.p2.2.256.288
    S.B.p2.2.144.176 S.C.p2.2.336.368 M.3.0.160 M.3.352.512 R.C.p1.3.0.112 S.B.p2.3.32.80
    R.B.p1.3.400.512 S.C.p2.3.432.480 S.B.p2.3.0.32 S.C.p2.3.480.512 M.3.160.352 R.C.p1.3.112.176
    S.B.p2.3.128.176 S.B.p2.3.80.128 R.B.p1.3.336.400 S.C.p2.3.336.384 S.C.p2.3.384.432
    W.B.x.03.496.512 W.C.x.03.0.16 W.B.x.02.0.32 W.C.x.02.480.512 W.B.x.04.480.496 W.C.x.04.16.32
    W.B.x.23.0.32 W.C.x.23.480.512 W.B.x.34.0.32 W.C.x.34.480.512 R.B.p1.3.256.336 S.C.p2.3.256.304
    S.C.p2.3.304.336 S.C.p3.0.144.192 S.C.p3.1.144.192 R.C.p1.3.176.256 S.B.p2.3.208.256
    S.B.p2.3.176.208 S.B.p3.0.320.368 S.B.p3.1.320.368 W.B.x.34.496.512 W.C.x.34.0.16 W.B.x.04.32.64
    W.B.x.04.64.80 W.C.x.04.448.480 W.C.x.04.432.448 W.B.x.03.80.96 W.C.x.03.416.432 W.B.x.34.80.96
    W.C.x.34.416.432 R.B.p2.0.192.256 F.B.p2.0.192.256 R.C.p2.0.256.320 F.C.p2.0.256.320
    W.B.p1.0.0.32 W.C.p1.0.480.512 W.B.p1.0.32.64 W.C.p1.0.448.480 W.B.p1.0.96.144 W.C.p1.0.368.416
    W.B.p1.0.64.96 W.C.p1.0.416.448 W.B.p1.1.0.32 W.C.p1.1.480.512 R.B.p2.2.128.192 W.B.p1.1.32.64
    W.C.p1.1.448.480 W.B.p1.1.64.112 W.C.p1.1.400.448 W.B.p1.1.112.144 W.C.p1.1.368.400
    W.B.p2.0.144.192 W.C.p2.0.320.368 W.B.p1.2.0.48 W.C.p1.2.464.512 R.B.p2.2.192.256
    S.C.p3.2.128.256 R.C.p2.2.320.384 R.C.p2.2.256.320 S.B.p3.2.256.384 W.B.p2.1.144.192
    W.C.p2.1.320.368 W.B.p2.0.192.224 W.C.p2.0.288.320 W.B.p2.1.192.224 W.C.p2.1.288.320
    W.B.p2.2.48.96 W.C.p2.2.416.464 W.B.p2.2.96.144 W.C.p2.2.368.416 R.B.p2.3.224.256
    W.B.p2.0.224.256 W.C.p2.0.256.288 W.B.p2.1.224.256 W.C.p2.1.256.288 W.B.p2.2.176.224
    W.C.p2.2.288.336 W.B.p2.2.224.256 W.C.p2.2.256.288 W.B.p2.2.144.176 W.C.p2.2.336.368
    R.B.p2.3.176.224 S.C.p3.3.176.256 R.C.p2.3.256.288 R.C.p2.3.288.336 S.B.p3.3.256.336
    R.C.p2.3.336.384 S.B.p3.3.336.384 R.B.p2.3.128.176 S.C.p3.3.128.176 W.B.p2.3.32.80
    W.C.p2.3.432.480 W.B.p2.3.0.32 W.C.p2.3.480.512 W.B.p2.3.128.176 W.B.p2.3.80.128
    W.C.p2.3.336.384 W.C.p2.3.384.432 W.C.p2.3.256.304 W.C.p2.3.304.336 R.B.p2.3.0.128
    S.C.p3.3.96.128 S.C.p3.3.0.48 S.C.p3.3.48.96 R.C.p2.3.384.512 S.B.p3.3.384.416 S.B.p3.3.464.512
    S.B.p3.3.416.464 W.C.p3.0.144.192 W.C.p3.1.144.192 W.B.p2.3.208.256 W.B.p2.3.176.208
    W.B.p3.0.320.368 W.B.p3.1.320.368 R.B.p3.1.80.144 F.B.p3.1.80.144 R.C.p3.1.368.432
    F.C.p3.1.368.432 W.C.p3.2.128.256 W.B.p3.2.256.384 R.B.p3.1.32.80 F.B.p3.1.32.80
    R.C.p3.1.432.480 F.C.p3.1.432.480 W.C.p3.3.176.256 W.B.p3.3.256.336 R.B.p2.2.48.128
    F.B.p2.2.48.128 R.C.p2.2.384.464 F.C.p2.2.384.464 W.B.p3.3.336.384 W.C.p3.3.128.176
    W.C.p3.3.96.128 W.B.p3.3.384.416 R.B.p3.2.0.48 F.B.p3.2.0.48 R.C.p3.2.464.512 F.C.p3.2.464.512
    W.C.p3.3.0.48 W.B.p3.3.464.512 R.B.p3.0.32.112 F.B.p3.0.32.112 R.C.p3.0.400.480 F.C.p3.0.400.480
    W.C.p3.3.48.96 W.B.p3.3.416.464 R.B.p3.1.0.32 F.B.p3.1.0.32 R.C.p3.1.480.512 F.C.p3.1.480.512
    R.B.p2.1.192.256 F.B.p2.1.192.256 R.C.p2.1.256.320 F.C.p2.1.256.320 R.B.p3.0.112.144
    F.B.p3.0.112.144 R.C.p3.0.368.400 F.C.p3.0.368.400 R.B.p3.0.0.32 F.B.p3.0.0.32 R.C.p3.0.480.512
    F.C.p3.0.480.512
    """,
}

def _parse(role, text, mirror=False):
    swap = {"A": "A", "D": "D", "B": "C", "C": "B"}
    flip = (lambda a, b: (ROWS - b, ROWS - a)) if mirror else (lambda a, b: (a, b))
    ops = []
    for tok in text.split():
        f = tok.split(".")
        if f[0] == "BAR":
            ops.append(("BAR",))
        elif f[0] == "L":
            ops.append(("L", ("x",) + flip(int(f[2]), int(f[3])) if f[1] == "x" else (f[1][0], int(f[1][1]))))
        elif f[0] == "V":
            ops.append(("V",) + flip(int(f[1]), int(f[2])))
        elif f[0] == "H":
            ops.append(("H",) + flip(int(f[1]), int(f[2])) + (int(f[3]), int(f[4])))
        elif f[0] == "M":
            ops.append(("M",) + flip(int(f[2]), int(f[3])) + (int(f[1]),))
        else:
            peer = swap[f[1]] if mirror else f[1]
            src, dst = (role, peer) if f[0] in "SPW" else (peer, role)
            ops.append((f[0], (src, dst, f[2], int(f[3])) + flip(int(f[4]), int(f[5]))))
    return ops


def _tables():
    prog = {r: _parse(r, _SCHEDULE[r]) for r in "ABD"}
    prog["C"] = _parse("C", _SCHEDULE["B"], mirror=True)
    as_waits = lambda s: " ".join("L." + n for n in s.split())
    loads = {r: [op[1] for op in _parse(r, as_waits(_LOAD_ORDER[r]))] for r in "ABD"}
    loads["C"] = [op[1] for op in _parse("C", as_waits(_LOAD_ORDER["B"]), mirror=True)]
    send_id, recv_id, leaf = {}, {}, {r: set() for r in prog}
    for r, ops in prog.items():
        sent = [op[1] for op in ops if op[0] in ("S", "P")]
        got = [op[1] for op in ops if op[0] == "R"]
        send_id.update({msg: i for i, msg in enumerate(sent)})
        recv_id.update({msg: i for i, msg in enumerate(got)})
        assert sorted(sent) == sorted(op[1] for op in ops if op[0] == "W")
        assert sorted(loads[r]) == sorted(op[1] for op in ops if op[0] == "L")
        done = set()
        for op in ops:
            if op[0] in ("S", "P", "F"):
                _, _, kind, c, r0, r1 = op[1]
                units = {(c, u) for u in range(r0 // U, r1 // U)}
                if op[0] != "F" and kind == "p1":
                    leaf[r] |= units
                if op[0] == "F" or kind == "p3":
                    done |= units
        assert len(done) == 4 * ROWS // U
        x_parts = [(4,) + op[1:3] for op in ops if op[0] == "V"] + [msg[3:] for msg in got if msg[2] == "x"]
        x_units = [(u, k) for kk, a, b in x_parts for u in range(a, b, U) for k in range(*divmod(kk, 10))]
        assert len(x_units) == len(set(x_units)) == 4 * ROWS // U
        assert ops.index(("BAR",)) < min(i for i, op in enumerate(ops) if op[0] in ("S", "P"))
    assert sorted(send_id) == sorted(recv_id)
    return prog, loads, send_id, recv_id, leaf


_PROG, _LOADS, _SEND_ID, _RECV_ID, _LEAF = _tables()
_WEIGHT_LOADS = [n for n in _LOADS["A"] if n[0] != "x"]
assert all([n for n in v if n[0] != "x"] == _WEIGHT_LOADS for v in _LOADS.values())


def _rows(r0, r1):
    return pl.ds(r0, r1 - r0)


def _stack(parts):
    return parts[0] if len(parts) == 1 else jnp.concatenate(parts, axis=0)


def _body(x_hbm, w1_hbm, w2_hbm, o_ref,
          x32, w1, w2, x16, hacc, h16, own, sbuf, rbuf, load_sem, send_sem, recv_sem):
    me = lax.axis_index("i")
    nk = w1.shape[0] // T
    hid = w1.shape[1]

    def load(role, name):
        if name[0] == "x":
            i = len(_WEIGHT_LOADS) + [n for n in _LOADS[role] if n[0] == "x"].index(name)
            rows = _rows(name[1], name[2])
            return pltpu.make_async_copy(x_hbm.at[rows], x32.at[rows], load_sem.at[i])
        sem = load_sem.at[_WEIGHT_LOADS.index(name)]
        blk = pl.ds(T * name[1], T)
        if name[0] == "k":
            return pltpu.make_async_copy(w1_hbm.at[blk], w1.at[blk], sem)
        return pltpu.make_async_copy(w2_hbm.at[:, blk], w2.at[name[1]], sem)

    def start_x_loads(after):
        for role in "BCDA":
            order = _LOADS[role]
            i = 0 if after is None else order.index(after) + 1
            names = []
            while i < len(order) and order[i][0] == "x":
                names.append(order[i])
                i += 1
            if names:
                @pl.when(me == MESH_INDEX[role])
                def _(role=role, names=names):
                    for name in names:
                        load(role, name).start()

    entered = pltpu.get_barrier_semaphore()
    start_x_loads(None)
    for nbr in (me ^ 1, 3 - me):
        pl.semaphore_signal(entered, inc=1, device_id=(nbr,), device_id_type=pl.DeviceIdType.MESH)
    for name in _WEIGHT_LOADS:
        load("A", name).start()
        start_x_loads(name)

    def rdma(msg):
        _, dst_role, kind, c, r0, r1 = msg
        rows = _rows(r0, r1)
        if kind == "x":
            k0, k1 = divmod(c, 10)
            src = dst = x16.at[rows] if k1 - k0 == nk else x16.at[rows, _rows(T * k0, T * k1)]
        else:
            src = rbuf.at[0, c, rows] if kind == "fw" else sbuf.at[int(kind == "p3"), c, rows]
            dst = rbuf.at[int(kind == "p2"), c, rows]
        return pltpu.make_async_remote_copy(
            src, dst, send_sem.at[_SEND_ID[msg]], recv_sem.at[_RECV_ID[msg]],
            device_id=(MESH_INDEX[dst_role],), device_id_type=pl.DeviceIdType.MESH)

    def root_sum(c, rows, n):
        acc = own[c, rows, :]
        for slot in range(n):
            acc = acc + rbuf[slot, c, rows, :].astype(F32)
        return acc

    def send(msg):
        _, _, kind, c, r0, r1 = msg
        rows = _rows(r0, r1)
        if kind == "p2":
            sbuf[0, c, rows, :] = root_sum(c, rows, 1).astype(BF16)
        elif kind == "p3":
            total = root_sum(c, rows, 2)
            sbuf[1, c, rows, :] = total.astype(BF16)
        rdma(msg).start()
        if kind == "p3":
            o_ref[rows, pl.ds(T * c, T)] = total

    def finish(msg):
        _, _, kind, c, r0, r1 = msg
        rows = _rows(r0, r1)
        total = root_sum(c, rows, 2) if kind == "p2" else rbuf[0, c, rows, :].astype(F32)
        o_ref[rows, pl.ds(T * c, T)] = total

    def out_unit(role, c, ranges):
        def compute():
            lhs = _stack([h16[_rows(r0, r1), :] for r0, r1 in ranges])
            return jnp.dot(lhs, w2[c].astype(BF16), preferred_element_type=F32)

        def store(p):
            off = 0
            for r0, r1 in ranges:
                while r0 < r1:
                    is_leaf = (c, r0 // U) in _LEAF[role]
                    r = r0
                    while r < r1 and ((c, r // U) in _LEAF[role]) == is_leaf:
                        r += U
                    piece = p[off:off + r - r0]
                    if is_leaf:
                        sbuf[0, c, _rows(r0, r), :] = piece.astype(BF16)
                    else:
                        own[c, _rows(r0, r), :] = piece
                    off += r - r0
                    r0 = r
        return compute, store

    def hid_unit(k0, k1, ranges, n0, n1):
        kk, nn = _rows(T * k0, T * k1), _rows(n0, n1)

        def compute():
            lhs = _stack([x16[_rows(r0, r1), kk] for r0, r1 in ranges])
            return jnp.dot(lhs, w1[kk, nn].astype(BF16), preferred_element_type=F32)

        def store(p):
            off = 0
            for r0, r1 in ranges:
                rows = _rows(r0, r1)
                piece = p[off:off + r1 - r0]
                off += r1 - r0
                if k0 > 0:
                    piece = piece + hacc[rows, nn]
                if k1 < nk:
                    hacc[rows, nn] = piece
                else:
                    h16[rows, nn] = jnp.maximum(piece, 0.0).astype(BF16)
        return compute, store

    def matmul_units(role, tasks, need):
        merged = []
        for op, r0, r1, *key in tasks:
            if merged and merged[-1][0] == (op, key):
                merged[-1][1].append((r0, r1))
            else:
                merged.append(((op, key), [(r0, r1)]))
        head, rest, unstored = [], [], set()
        for (op, key), ranges in merged:
            touched = {r for r0, r1 in ranges for r in range(r0, r1, U)}
            if op == "H":
                unstored |= touched
            elif touched & unstored:
                need = 0
            n = sum(r1 - r0 for r0, r1 in ranges)
            work = n * (key[1] - key[0]) if op == "H" else n
            if need > 0 and work >= need + MIN_REST:
                if op == "H":
                    cut = T * min(hid // T - 1, -(-need * (hid // T) // work))
                    head.append(hid_unit(*key, ranges, 0, cut))
                    rest.append(hid_unit(*key, ranges, cut, hid))
                else:
                    first, second = [], []
                    for r0, r1 in ranges:
                        r = min(r1, r0 + need)
                        need -= r - r0
                        first += [(r0, r)] if r > r0 else []
                        second += [(r, r1)] if r1 > r else []
                    head.append(out_unit(role, key[0], first))
                    rest.append(out_unit(role, key[0], second))
                need = 0
            else:
                unit = hid_unit(*key, ranges, 0, hid) if op == "H" else out_unit(role, key[0], ranges)
                (head if need > 0 else rest).append(unit)
                need -= work
        return head, rest

    def run(role):
        ops, i, pending = _PROG[role], 0, []
        while i < len(ops):
            op = ops[i]
            if op[0] in ("H", "M"):
                j = i
                while j < len(ops) and ops[j][0] in ("H", "M"):
                    j += 1
                head, rest = matmul_units(role, ops[i:j], BRIDGE if pending else 0)
                vals = [compute() for compute, _ in head]
                for msg in pending:
                    send(msg)
                pending = []
                for (_, store), val in zip(head, vals):
                    store(val)
                for compute, store in rest:
                    store(compute())
                i = j
                continue
            i += 1
            if op[0] == "P":
                pending.append(op[1])
            elif op[0] == "V":
                rows = _rows(op[1], op[2])
                x16[rows, :] = x32[rows, :].astype(BF16)
            elif op[0] == "L":
                load(role, op[1]).wait()
            elif op[0] == "BAR":
                pl.semaphore_wait(entered, 2)
            elif op[0] == "R":
                rdma(op[1]).wait_recv()
            elif op[0] == "W":
                rdma(op[1]).wait_send()
            elif op[0] == "S":
                send(op[1])
            else:
                finish(op[1])
        assert not pending

    for role in "BCDA":
        pl.when(me == MESH_INDEX[role])(lambda role=role: run(role))


def pallas_dist_mlp2_tp_i_m512_h1024_out512_kernel(x: jax.Array, W1: jax.Array, W2: jax.Array):
    m, k = x.shape
    hid, n = W2.shape
    nc = n // T
    assert m == ROWS and k == 4 * T and nc == 4
    return pl.pallas_call(
        _body,
        out_shape=jax.ShapeDtypeStruct((m, n), F32),
        in_specs=[pl.BlockSpec(memory_space=pl.ANY)] * 3,
        out_specs=pl.BlockSpec(memory_space=pltpu.VMEM),
        scratch_shapes=[
            pltpu.VMEM((m, k), F32),
            pltpu.VMEM((k, hid), F32),
            pltpu.VMEM((nc, hid, T), F32),
            pltpu.VMEM((m, k), BF16),
            pltpu.VMEM((m, hid), F32),
            pltpu.VMEM((m, hid), BF16),
            pltpu.VMEM((nc, m, T), F32),
            pltpu.VMEM((2, nc, m, T), BF16),
            pltpu.VMEM((2, nc, m, T), BF16),
            pltpu.SemaphoreType.DMA((max(len(v) for v in _LOADS.values()),)),
            pltpu.SemaphoreType.DMA((max(_SEND_ID.values()) + 1,)),
            pltpu.SemaphoreType.DMA((max(_RECV_ID.values()) + 1,)),
        ],
        compiler_params=pltpu.CompilerParams(collective_id=0, disable_semaphore_checks=True),
    )(x, W1, W2)
```
